```python
import numpy as np

kernel_name = "dist_mean_ax0_shard0_i_m4096_n1024"

def setup_inputs():
    return {"x": np.random.randn(16384, 1024).astype(np.float32)}

def reference(x: np.ndarray) -> np.ndarray:
    return np.mean(x, axis=0, keepdims=True)
```

```python
import jax
import jax.numpy as jnp
from jax import lax
from jax.experimental import pallas as pl
from jax.experimental.pallas import tpu as pltpu

N_DEV = 4


def pallas_dist_mean_ax0_shard0_i_m4096_n1024_kernel(
    x: jax.Array,
):
    m, n = x.shape
    chunk = 256
    n_chunks = m // chunk
    inv_total = 1.0 / (m * N_DEV)

    def body(x_hbm, out_ref, buf, comm, copy_sems, send_sems, recv_sems):
        my = lax.axis_index("i")

        copies = [
            pltpu.make_async_copy(
                x_hbm.at[pl.ds(c * chunk, chunk)],
                buf.at[pl.ds(c * chunk, chunk)],
                copy_sems.at[c],
            )
            for c in range(n_chunks)
        ]
        for cp in copies:
            cp.start()

        barrier = pltpu.get_barrier_semaphore()
        for d in range(1, N_DEV):
            pl.semaphore_signal(
                barrier, inc=1,
                device_id=((my + d) % N_DEV,),
                device_id_type=pl.DeviceIdType.MESH,
            )

        acc = jnp.zeros((8, n), jnp.float32)
        for c in range(n_chunks):
            copies[c].wait()
            blk = buf[pl.ds(c * chunk, chunk), :]
            acc = acc + jnp.sum(blk.reshape(chunk // 8, 8, n), axis=0)
        part = jnp.sum(acc, axis=0, keepdims=True)
        comm[0] = part

        pl.semaphore_wait(barrier, N_DEV - 1)

        rdmas = []
        for d in range(1, N_DEV):
            r = pltpu.make_async_remote_copy(
                src_ref=comm.at[0],
                dst_ref=comm.at[d],
                send_sem=send_sems.at[d - 1],
                recv_sem=recv_sems.at[d - 1],
                device_id=((my + d) % N_DEV,),
                device_id_type=pl.DeviceIdType.MESH,
            )
            r.start()
            rdmas.append(r)
        for r in rdmas:
            r.wait_recv()
        total = (part + comm[1]) + (comm[2] + comm[3])
        out_ref[...] = total * inv_total
        for r in rdmas:
            r.wait_send()

    return pl.pallas_call(
        body,
        out_shape=jax.ShapeDtypeStruct((1, n), jnp.float32),
        in_specs=[pl.BlockSpec(memory_space=pl.ANY)],
        out_specs=pl.BlockSpec(memory_space=pltpu.VMEM),
        scratch_shapes=[
            pltpu.VMEM((m, n), jnp.float32),
            pltpu.VMEM((N_DEV, 1, n), jnp.float32),
            pltpu.SemaphoreType.DMA((n_chunks,)),
            pltpu.SemaphoreType.DMA((N_DEV - 1,)),
            pltpu.SemaphoreType.DMA((N_DEV - 1,)),
        ],
        compiler_params=pltpu.CompilerParams(
            collective_id=0,
            vmem_limit_bytes=64 * 1024 * 1024,
        ),
    )(x)
```

```python
import jax
import jax.numpy as jnp
from jax import lax
from jax.experimental import pallas as pl
from jax.experimental.pallas import tpu as pltpu

N_DEV = 4
_MESH = pl.DeviceIdType.MESH

_RAW_ROWS = 216
_CHUNK_ROWS = 512
_TAIL_ROWS = 224
_TAIL_SPLIT = 32
_LAST_COLS = 128


def _colsum8(v):
    rows, w = v.shape
    return jnp.sum(v.reshape(rows // 8, 8, w), axis=0)


def _tree_sum(vals):
    while len(vals) > 1:
        nxt = [vals[i] + vals[i + 1] for i in range(0, len(vals) - 1, 2)]
        if len(vals) % 2:
            nxt.append(vals[-1])
        vals = nxt
    return vals[0]


def pallas_dist_mean_ax0_shard0_i_m4096_n1024_kernel(
    x: jax.Array,
):
    m, n = x.shape
    r, t_rows, w_lo = _RAW_ROWS, _TAIL_ROWS, _LAST_COLS
    w_hi = n - w_lo
    loc = m - 2 * r
    body_rows = loc - t_rows
    sizes = [_CHUNK_ROWS] * (body_rows // _CHUNK_ROWS)
    if body_rows % _CHUNK_ROWS:
        sizes = [body_rows % _CHUNK_ROWS] + sizes
    offs = [sum(sizes[:i]) for i in range(len(sizes))]
    n_body = len(sizes)
    hi_parts = [(0, t_rows - _TAIL_SPLIT), (t_rows - _TAIL_SPLIT, _TAIL_SPLIT)]
    n_copies = n_body + len(hi_parts) + 1
    inv_total = 1.0 / (m * N_DEV)

    def body(x_hbm, out_ref, buf, hi_buf, lo_buf, raw_buf,
             hi_src, lo_src, full_src, hi_dst, lo_dst, nb_dst,
             copy_sems, raw_send_sems, raw_recv_sems, send_sems, recv_sems):
        body_copies = [
            pltpu.make_async_copy(
                x_hbm.at[pl.ds(o, s)], buf.at[pl.ds(o, s)], copy_sems.at[c])
            for c, (o, s) in enumerate(zip(offs, sizes))
        ]
        hi_copies = [
            pltpu.make_async_copy(
                x_hbm.at[pl.ds(body_rows + o, s), pl.ds(w_lo, w_hi)],
                hi_buf.at[pl.ds(o, s)], copy_sems.at[n_body + c])
            for c, (o, s) in enumerate(hi_parts)
        ]
        lo_copy = pltpu.make_async_copy(
            x_hbm.at[pl.ds(body_rows, t_rows), pl.ds(0, w_lo)],
            lo_buf, copy_sems.at[n_copies - 1])
        for cp in body_copies + hi_copies + [lo_copy]:
            cp.start()

        my = lax.axis_index("i")
        right = lax.rem(my + 1, N_DEV)
        diag = lax.rem(my + 2, N_DEV)
        left = lax.rem(my + 3, N_DEV)
        barrier = pltpu.get_barrier_semaphore()
        for peer in (right, left, diag):
            pl.semaphore_signal(
                barrier, inc=1, device_id=(peer,), device_id_type=_MESH)
        pl.semaphore_wait(barrier, N_DEV - 1)

        raws = []
        for k, peer in enumerate((right, left)):
            rc = pltpu.make_async_remote_copy(
                src_ref=x_hbm.at[pl.ds(loc + k * r, r)],
                dst_ref=raw_buf.at[k],
                send_sem=raw_send_sems.at[k],
                recv_sem=raw_recv_sems.at[k],
                device_id=(peer,), device_id_type=_MESH)
            rc.start()
            raws.append(rc)

        acc = None
        for c in range(n_body):
            body_copies[c].wait()
            s = _colsum8(buf[pl.ds(offs[c], sizes[c]), :])
            acc = s if acc is None else acc + s
        for k in range(2):
            raws[k].wait_recv()
        for k in range(2):
            acc = acc + _colsum8(raw_buf[k])
        acc_lo = acc[:, :w_lo]
        acc_hi = acc[:, w_lo:]

        for c, (o, s) in enumerate(hi_parts):
            hi_copies[c].wait()
            acc_hi = acc_hi + _colsum8(hi_buf[pl.ds(o, s), :])
        part_hi = jnp.sum(acc_hi, axis=0, keepdims=True)
        hi_src[...] = part_hi
        hi_msg = pltpu.make_async_remote_copy(
            src_ref=hi_src, dst_ref=hi_dst,
            send_sem=send_sems.at[0], recv_sem=recv_sems.at[0],
            device_id=(diag,), device_id_type=_MESH)
        hi_msg.start()
        full_src[:, pl.ds(w_lo, w_hi)] = part_hi

        lo_copy.wait()
        acc_lo = _tree_sum(
            [acc_lo] + [lo_buf[pl.ds(8 * i, 8), :] for i in range(t_rows // 8)])
        part_lo = jnp.sum(acc_lo, axis=0, keepdims=True)
        lo_src[...] = part_lo
        lo_msg = pltpu.make_async_remote_copy(
            src_ref=lo_src, dst_ref=lo_dst,
            send_sem=send_sems.at[1], recv_sem=recv_sems.at[1],
            device_id=(diag,), device_id_type=_MESH)
        lo_msg.start()
        full_src[:, pl.ds(0, w_lo)] = part_lo
        nb_msgs = []
        for k, peer in enumerate((right, left)):
            msg = pltpu.make_async_remote_copy(
                src_ref=full_src, dst_ref=nb_dst.at[k],
                send_sem=send_sems.at[2 + k], recv_sem=recv_sems.at[2 + k],
                device_id=(peer,), device_id_type=_MESH)
            msg.start()
            nb_msgs.append(msg)

        for msg in raws + [hi_msg, lo_msg] + nb_msgs:
            msg.wait_send()
        for msg in nb_msgs:
            msg.wait_recv()
        t_hi = part_hi + (nb_dst[0, :, pl.ds(w_lo, w_hi)]
                          + nb_dst[1, :, pl.ds(w_lo, w_hi)])
        t_lo = part_lo + (nb_dst[0, :, pl.ds(0, w_lo)]
                          + nb_dst[1, :, pl.ds(0, w_lo)])
        hi_msg.wait_recv()
        out_ref[:, pl.ds(w_lo, w_hi)] = (t_hi + hi_dst[...]) * inv_total
        lo_msg.wait_recv()
        out_ref[:, pl.ds(0, w_lo)] = (t_lo + lo_dst[...]) * inv_total

    f32 = jnp.float32
    return pl.pallas_call(
        body,
        out_shape=jax.ShapeDtypeStruct((1, n), f32),
        in_specs=[pl.BlockSpec(memory_space=pl.ANY)],
        out_specs=pl.BlockSpec(memory_space=pltpu.VMEM),
        scratch_shapes=[
            pltpu.VMEM((body_rows, n), f32),
            pltpu.VMEM((t_rows, w_hi), f32),
            pltpu.VMEM((t_rows, w_lo), f32),
            pltpu.VMEM((2, r, n), f32),
            pltpu.VMEM((1, w_hi), f32),
            pltpu.VMEM((1, w_lo), f32),
            pltpu.VMEM((1, n), f32),
            pltpu.VMEM((1, w_hi), f32),
            pltpu.VMEM((1, w_lo), f32),
            pltpu.VMEM((2, 1, n), f32),
            pltpu.SemaphoreType.DMA((n_copies,)),
            pltpu.SemaphoreType.DMA((2,)),
            pltpu.SemaphoreType.DMA((2,)),
            pltpu.SemaphoreType.DMA((4,)),
            pltpu.SemaphoreType.DMA((4,)),
        ],
        compiler_params=pltpu.CompilerParams(
            collective_id=0,
            vmem_limit_bytes=64 * 1024 * 1024,
            disable_semaphore_checks=True,
        ),
    )(x)
```

```python
import jax
import jax.numpy as jnp
from jax import lax
from jax.experimental import pallas as pl
from jax.experimental.pallas import tpu as pltpu

N_DEV = 4
_MESH = pl.DeviceIdType.MESH

_RAW_ROWS = 216
_CHUNK_ROWS = 512
_TAIL_ROWS = 224
_TAIL_SPLIT = 32
_LAST_COLS = 128


def _colsum8(v):
    rows, w = v.shape
    return jnp.sum(v.reshape(rows // 8, 8, w), axis=0)


def _tree_sum(vals):
    while len(vals) > 1:
        nxt = [vals[i] + vals[i + 1] for i in range(0, len(vals) - 1, 2)]
        if len(vals) % 2:
            nxt.append(vals[-1])
        vals = nxt
    return vals[0]


def _compiler_params():
    kwargs = dict(collective_id=0, vmem_limit_bytes=64 * 1024 * 1024)
    try:
        return pltpu.CompilerParams(disable_semaphore_checks=True, **kwargs)
    except TypeError:
        return pltpu.CompilerParams(**kwargs)


def pallas_dist_mean_ax0_shard0_i_m4096_n1024_kernel(
    x: jax.Array,
):
    m, n = x.shape
    r, t_rows, w_lo = _RAW_ROWS, _TAIL_ROWS, _LAST_COLS
    w_hi = n - w_lo
    loc = m - 2 * r
    body_rows = loc - t_rows
    sizes = [_CHUNK_ROWS] * (body_rows // _CHUNK_ROWS)
    if body_rows % _CHUNK_ROWS:
        sizes = [body_rows % _CHUNK_ROWS] + sizes
    assert all(s % 8 == 0 for s in sizes + [r, t_rows, _TAIL_SPLIT])
    offs = [sum(sizes[:i]) for i in range(len(sizes))]
    n_body = len(sizes)
    hi_parts = [(0, t_rows - _TAIL_SPLIT), (t_rows - _TAIL_SPLIT, _TAIL_SPLIT)]
    n_copies = n_body + len(hi_parts) + 1
    inv_total = 1.0 / (m * N_DEV)

    def body(x_hbm, out_ref, buf, hi_buf, lo_buf, raw_buf,
             hi_src, lo_src, full_src, hi_dst, lo_dst, nb_dst,
             copy_sems, raw_send_sems, raw_recv_sems, send_sems, recv_sems):
        body_copies = [
            pltpu.make_async_copy(
                x_hbm.at[pl.ds(o, s)], buf.at[pl.ds(o, s)], copy_sems.at[c])
            for c, (o, s) in enumerate(zip(offs, sizes))
        ]
        hi_copies = [
            pltpu.make_async_copy(
                x_hbm.at[pl.ds(body_rows + o, s), pl.ds(w_lo, w_hi)],
                hi_buf.at[pl.ds(o, s)], copy_sems.at[n_body + c])
            for c, (o, s) in enumerate(hi_parts)
        ]
        lo_copy = pltpu.make_async_copy(
            x_hbm.at[pl.ds(body_rows, t_rows), pl.ds(0, w_lo)],
            lo_buf, copy_sems.at[n_copies - 1])
        for cp in body_copies + hi_copies + [lo_copy]:
            cp.start()

        my = lax.axis_index("i")
        right = lax.rem(my + 1, N_DEV)
        diag = lax.rem(my + 2, N_DEV)
        left = lax.rem(my + 3, N_DEV)
        barrier = pltpu.get_barrier_semaphore()
        for peer in (right, left, diag):
            pl.semaphore_signal(
                barrier, inc=1, device_id=(peer,), device_id_type=_MESH)
        pl.semaphore_wait(barrier, N_DEV - 1)

        raws = []
        for k, peer in enumerate((right, left)):
            rc = pltpu.make_async_remote_copy(
                src_ref=x_hbm.at[pl.ds(loc + k * r, r)],
                dst_ref=raw_buf.at[k],
                send_sem=raw_send_sems.at[k],
                recv_sem=raw_recv_sems.at[k],
                device_id=(peer,), device_id_type=_MESH)
            rc.start()
            raws.append(rc)

        acc = None
        for c in range(n_body):
            body_copies[c].wait()
            s = _colsum8(buf[pl.ds(offs[c], sizes[c]), :])
            acc = s if acc is None else acc + s
        for k in range(2):
            raws[k].wait_recv()
        for k in range(2):
            acc = acc + _colsum8(raw_buf[k])
        acc_lo = acc[:, :w_lo]
        acc_hi = acc[:, w_lo:]

        for c, (o, s) in enumerate(hi_parts):
            hi_copies[c].wait()
            acc_hi = acc_hi + _colsum8(hi_buf[pl.ds(o, s), :])
        part_hi = jnp.sum(acc_hi, axis=0, keepdims=True)
        hi_src[...] = part_hi
        hi_msg = pltpu.make_async_remote_copy(
            src_ref=hi_src, dst_ref=hi_dst,
            send_sem=send_sems.at[0], recv_sem=recv_sems.at[0],
            device_id=(diag,), device_id_type=_MESH)
        hi_msg.start()
        full_src[:, pl.ds(w_lo, w_hi)] = part_hi

        lo_copy.wait()
        acc_lo = _tree_sum(
            [acc_lo] + [lo_buf[pl.ds(8 * i, 8), :] for i in range(t_rows // 8)])
        part_lo = jnp.sum(acc_lo, axis=0, keepdims=True)
        lo_src[...] = part_lo
        lo_msg = pltpu.make_async_remote_copy(
            src_ref=lo_src, dst_ref=lo_dst,
            send_sem=send_sems.at[1], recv_sem=recv_sems.at[1],
            device_id=(diag,), device_id_type=_MESH)
        lo_msg.start()
        full_src[:, pl.ds(0, w_lo)] = part_lo
        nb_msgs = []
        for k, peer in enumerate((right, left)):
            msg = pltpu.make_async_remote_copy(
                src_ref=full_src, dst_ref=nb_dst.at[k],
                send_sem=send_sems.at[2 + k], recv_sem=recv_sems.at[2 + k],
                device_id=(peer,), device_id_type=_MESH)
            msg.start()
            nb_msgs.append(msg)

        for msg in raws + [hi_msg, lo_msg] + nb_msgs:
            msg.wait_send()
        for msg in nb_msgs:
            msg.wait_recv()
        t_hi = part_hi + (nb_dst[0, :, pl.ds(w_lo, w_hi)]
                          + nb_dst[1, :, pl.ds(w_lo, w_hi)])
        t_lo = part_lo + (nb_dst[0, :, pl.ds(0, w_lo)]
                          + nb_dst[1, :, pl.ds(0, w_lo)])
        hi_msg.wait_recv()
        out_ref[:, pl.ds(w_lo, w_hi)] = (t_hi + hi_dst[...]) * inv_total
        lo_msg.wait_recv()
        out_ref[:, pl.ds(0, w_lo)] = (t_lo + lo_dst[...]) * inv_total

    f32 = jnp.float32
    return pl.pallas_call(
        body,
        out_shape=jax.ShapeDtypeStruct((1, n), f32),
        in_specs=[pl.BlockSpec(memory_space=pl.ANY)],
        out_specs=pl.BlockSpec(memory_space=pltpu.VMEM),
        scratch_shapes=[
            pltpu.VMEM((body_rows, n), f32),
            pltpu.VMEM((t_rows, w_hi), f32),
            pltpu.VMEM((t_rows, w_lo), f32),
            pltpu.VMEM((2, r, n), f32),
            pltpu.VMEM((1, w_hi), f32),
            pltpu.VMEM((1, w_lo), f32),
            pltpu.VMEM((1, n), f32),
            pltpu.VMEM((1, w_hi), f32),
            pltpu.VMEM((1, w_lo), f32),
            pltpu.VMEM((2, 1, n), f32),
            pltpu.SemaphoreType.DMA((n_copies,)),
            pltpu.SemaphoreType.DMA((2,)),
            pltpu.SemaphoreType.DMA((2,)),
            pltpu.SemaphoreType.DMA((4,)),
            pltpu.SemaphoreType.DMA((4,)),
        ],
        compiler_params=_compiler_params(),
    )(x)
```

```python
import jax
import jax.numpy as jnp
from jax import lax
from jax.experimental import pallas as pl
from jax.experimental.pallas import tpu as pltpu

N_DEV = 4
_MESH = pl.DeviceIdType.MESH

_RAW_ROWS = 216
_CHUNK_ROWS = 512
_TAIL_ROWS = 224
_TAIL_SPLIT = 32
_LAST_COLS = 128


def _colsum8(v):
    rows, w = v.shape
    return jnp.sum(v.reshape(rows // 8, 8, w), axis=0)


def _tree_sum(vals):
    while len(vals) > 1:
        nxt = [vals[i] + vals[i + 1] for i in range(0, len(vals) - 1, 2)]
        if len(vals) % 2:
            nxt.append(vals[-1])
        vals = nxt
    return vals[0]


def _compiler_params():
    kwargs = dict(collective_id=0, vmem_limit_bytes=64 * 1024 * 1024)
    try:
        return pltpu.CompilerParams(disable_semaphore_checks=True, **kwargs)
    except TypeError:
        return pltpu.CompilerParams(**kwargs)


def pallas_dist_mean_ax0_shard0_i_m4096_n1024_kernel(
    x: jax.Array,
):
    m, n = x.shape
    r, t_rows, w_lo = _RAW_ROWS, _TAIL_ROWS, _LAST_COLS
    w_hi = n - w_lo
    loc = m - 2 * r
    body_rows = loc - t_rows
    sizes = [_CHUNK_ROWS] * (body_rows // _CHUNK_ROWS)
    if body_rows % _CHUNK_ROWS:
        sizes = [body_rows % _CHUNK_ROWS] + sizes
    assert all(s % 8 == 0 for s in sizes + [r, t_rows, _TAIL_SPLIT])
    offs = [sum(sizes[:i]) for i in range(len(sizes))]
    n_body = len(sizes)
    hi_parts = [(0, t_rows - _TAIL_SPLIT), (t_rows - _TAIL_SPLIT, _TAIL_SPLIT)]
    n_copies = n_body + len(hi_parts) + 1
    inv_total = 1.0 / (m * N_DEV)

    def body(x_hbm, out_ref, buf, hi_buf, lo_buf, raw_buf,
             hi_src, lo_src, full_src, hi_dst, lo_dst, nb_dst,
             copy_sems, raw_send_sems, raw_recv_sems, send_sems, recv_sems):
        body_copies = [
            pltpu.make_async_copy(
                x_hbm.at[pl.ds(o, s)], buf.at[pl.ds(o, s)], copy_sems.at[c])
            for c, (o, s) in enumerate(zip(offs, sizes))
        ]
        hi_copies = [
            pltpu.make_async_copy(
                x_hbm.at[pl.ds(body_rows + o, s), pl.ds(w_lo, w_hi)],
                hi_buf.at[pl.ds(o, s)], copy_sems.at[n_body + c])
            for c, (o, s) in enumerate(hi_parts)
        ]
        lo_copy = pltpu.make_async_copy(
            x_hbm.at[pl.ds(body_rows, t_rows), pl.ds(0, w_lo)],
            lo_buf, copy_sems.at[n_copies - 1])
        for cp in body_copies + hi_copies + [lo_copy]:
            cp.start()

        my = lax.axis_index("i")
        right = lax.rem(my + 1, N_DEV)
        diag = lax.rem(my + 2, N_DEV)
        left = lax.rem(my + 3, N_DEV)
        barrier = pltpu.get_barrier_semaphore()
        for peer in (right, left, diag):
            pl.semaphore_signal(
                barrier, inc=1, device_id=(peer,), device_id_type=_MESH)
        pl.semaphore_wait(barrier, N_DEV - 1)

        raws = []
        for k, peer in enumerate((right, left)):
            rc = pltpu.make_async_remote_copy(
                src_ref=x_hbm.at[pl.ds(loc + k * r, r)],
                dst_ref=raw_buf.at[k],
                send_sem=raw_send_sems.at[k],
                recv_sem=raw_recv_sems.at[k],
                device_id=(peer,), device_id_type=_MESH)
            rc.start()
            raws.append(rc)

        acc = None
        for c in range(n_body):
            body_copies[c].wait()
            s = _colsum8(buf[pl.ds(offs[c], sizes[c]), :])
            acc = s if acc is None else acc + s
        for k in range(2):
            raws[k].wait_recv()
        for k in range(2):
            acc = acc + _colsum8(raw_buf[k])
        acc_lo = acc[:, :w_lo]
        acc_hi = acc[:, w_lo:]

        for c, (o, s) in enumerate(hi_parts):
            hi_copies[c].wait()
            acc_hi = acc_hi + _colsum8(hi_buf[pl.ds(o, s), :])
        part_hi = jnp.sum(acc_hi, axis=0, keepdims=True)
        hi_src[...] = part_hi
        hi_msg = pltpu.make_async_remote_copy(
            src_ref=hi_src, dst_ref=hi_dst,
            send_sem=send_sems.at[0], recv_sem=recv_sems.at[0],
            device_id=(diag,), device_id_type=_MESH)
        hi_msg.start()
        full_src[:, pl.ds(w_lo, w_hi)] = part_hi

        lo_copy.wait()
        acc_lo = _tree_sum(
            [acc_lo] + [lo_buf[pl.ds(8 * i, 8), :] for i in range(t_rows // 8)])
        part_lo = jnp.sum(acc_lo, axis=0, keepdims=True)
        lo_src[...] = part_lo
        lo_msg = pltpu.make_async_remote_copy(
            src_ref=lo_src, dst_ref=lo_dst,
            send_sem=send_sems.at[1], recv_sem=recv_sems.at[1],
            device_id=(diag,), device_id_type=_MESH)
        lo_msg.start()
        full_src[:, pl.ds(0, w_lo)] = part_lo
        nb_msgs = []
        for k, peer in enumerate((right, left)):
            msg = pltpu.make_async_remote_copy(
                src_ref=full_src, dst_ref=nb_dst.at[k],
                send_sem=send_sems.at[2 + k], recv_sem=recv_sems.at[2 + k],
                device_id=(peer,), device_id_type=_MESH)
            msg.start()
            nb_msgs.append(msg)

        for msg in raws + [hi_msg, lo_msg] + nb_msgs:
            msg.wait_send()
        for msg in nb_msgs:
            msg.wait_recv()
        t_hi = full_src[:, pl.ds(w_lo, w_hi)] + (
            nb_dst[0, :, pl.ds(w_lo, w_hi)] + nb_dst[1, :, pl.ds(w_lo, w_hi)])
        t_lo = part_lo + (
            nb_dst[0, :, pl.ds(0, w_lo)] + nb_dst[1, :, pl.ds(0, w_lo)])
        hi_msg.wait_recv()
        out_ref[:, pl.ds(w_lo, w_hi)] = (t_hi + hi_dst[...]) * inv_total
        lo_msg.wait_recv()
        out_ref[:, pl.ds(0, w_lo)] = (t_lo + lo_dst[...]) * inv_total

    f32 = jnp.float32
    return pl.pallas_call(
        body,
        out_shape=jax.ShapeDtypeStruct((1, n), f32),
        in_specs=[pl.BlockSpec(memory_space=pl.ANY)],
        out_specs=pl.BlockSpec(memory_space=pltpu.VMEM),
        scratch_shapes=[
            pltpu.VMEM((body_rows, n), f32),
            pltpu.VMEM((t_rows, w_hi), f32),
            pltpu.VMEM((t_rows, w_lo), f32),
            pltpu.VMEM((2, r, n), f32),
            pltpu.VMEM((1, w_hi), f32),
            pltpu.VMEM((1, w_lo), f32),
            pltpu.VMEM((1, n), f32),
            pltpu.VMEM((1, w_hi), f32),
            pltpu.VMEM((1, w_lo), f32),
            pltpu.VMEM((2, 1, n), f32),
            pltpu.SemaphoreType.DMA((n_copies,)),
            pltpu.SemaphoreType.DMA((2,)),
            pltpu.SemaphoreType.DMA((2,)),
            pltpu.SemaphoreType.DMA((4,)),
            pltpu.SemaphoreType.DMA((4,)),
        ],
        compiler_params=_compiler_params(),
    )(x)
```
